```python
import numpy as np

kernel_name = "dist_sum_ax0_xy_m2048_n1024"

def setup_inputs():
    return {"x": np.random.randn(4096, 2048).astype(np.float32)}

def reference(x: np.ndarray) -> np.ndarray:
    return np.sum(x, axis=0, keepdims=True)
```

```python
import jax
import jax.numpy as jnp
from jax import lax
from jax.experimental import pallas as pl
from jax.experimental.pallas import tpu as pltpu

N_CHUNKS = 8


def pallas_dist_sum_ax0_xy_m2048_n1024_kernel(x: jax.Array):
    m, n = x.shape
    rows = m // N_CHUNKS

    def body(x_hbm, out_ref, buf, mine, theirs, load_sems, send_sem, recv_sem):
        loads = [
            pltpu.make_async_copy(
                x_hbm.at[pl.ds(c * rows, rows)], buf.at[pl.ds(c * rows, rows)], load_sems.at[c]
            )
            for c in range(N_CHUNKS)
        ]
        for ld in loads:
            ld.start()
        my_x = lax.axis_index("x")
        my_y = lax.axis_index("y")
        peer = (1 - my_x, my_y)
        barrier = pltpu.get_barrier_semaphore()
        pl.semaphore_signal(barrier, inc=1, device_id=peer, device_id_type=pl.DeviceIdType.MESH)

        acc = jnp.zeros((8, n), jnp.float32)
        for c in range(N_CHUNKS):
            loads[c].wait()
            acc = acc + buf[pl.ds(c * rows, rows), :].reshape(rows // 8, 8, n).sum(axis=0)
        mine[...] = acc.sum(axis=0, keepdims=True)

        pl.semaphore_wait(barrier, 1)
        rdma = pltpu.make_async_remote_copy(
            src_ref=mine, dst_ref=theirs, send_sem=send_sem, recv_sem=recv_sem,
            device_id=peer, device_id_type=pl.DeviceIdType.MESH,
        )
        rdma.start()
        rdma.wait()
        out_ref[...] = mine[...] + theirs[...]

    return pl.pallas_call(
        body,
        out_shape=jax.ShapeDtypeStruct((1, n), jnp.float32),
        in_specs=[pl.BlockSpec(memory_space=pl.ANY)],
        out_specs=pl.BlockSpec(memory_space=pltpu.VMEM),
        scratch_shapes=[
            pltpu.VMEM((m, n), jnp.float32),
            pltpu.VMEM((1, n), jnp.float32),
            pltpu.VMEM((1, n), jnp.float32),
            pltpu.SemaphoreType.DMA((N_CHUNKS,)),
            pltpu.SemaphoreType.DMA,
            pltpu.SemaphoreType.DMA,
        ],
        compiler_params=pltpu.CompilerParams(collective_id=0, vmem_limit_bytes=32 * 1024 * 1024),
    )(x)
```

```python
import jax
import jax.numpy as jnp
from jax import lax
from jax.experimental import pallas as pl
from jax.experimental.pallas import tpu as pltpu

_SUB = 8
_LANES = 128

_ORDER_BITS = (7, 6, 5, 1, 0, 2, 3, 4)
_PREFILL = 30
_TAIL = 24
_BULK_LAST = 24
_WIDE_LAST = 2
_NARROW_LAST = 2
_UNROLL = 8


def _read_order(bits):
    order = []
    for slot in range(1 << len(bits)):
        order.append(sum(((slot >> k) & 1) << b for k, b in enumerate(bits)))
    return order


def _tree_sum(vals):
    vals = list(vals)
    while len(vals) > 1:
        pairs = [vals[i] + vals[i + 1] for i in range(0, len(vals) - 1, 2)]
        vals = pairs + (vals[-1:] if len(vals) % 2 else [])
    return vals[0]


def pallas_dist_sum_ax0_xy_m2048_n1024_kernel(x: jax.Array):
    m, n = x.shape
    order = _read_order(_ORDER_BITS)
    assert m == len(order) * _SUB and n % _LANES == 0
    wide = n - _LANES
    n_full = len(order) - _TAIL

    full_parts = (n_full - _BULK_LAST, _BULK_LAST)
    wide_parts = (_TAIL - _WIDE_LAST, _WIDE_LAST)
    narrow_parts = (_TAIL - _NARROW_LAST, _NARROW_LAST)

    loads = []
    sem = 0
    for which, parts, first in ((0, full_parts, 0), (1, wide_parts, n_full), (2, narrow_parts, n_full)):
        slot = 0
        for count in parts:
            for _ in range(count):
                loads.append((which, order[first + slot], slot, sem))
                slot += 1
            sem += 1
    n_sems = sem

    pairs = (len(loads) - _PREFILL) // 2
    low = [loads[2 * i] for i in range(pairs)] + loads[2 * pairs:]
    high = [loads[2 * i + 1] for i in range(pairs)]
    starts = [(ld, 1) for ld in low[:_PREFILL]]
    for i in range(pairs):
        starts += [(high[i], 0), (low[_PREFILL + i], 1)]
    starts += [(ld, 1) for ld in low[_PREFILL + pairs:]]

    def body(x_hbm, out_ref, full_buf, wide_buf, narrow_buf, mine, theirs, load_sems, send_sems, recv_sems):
        bufs = (full_buf, wide_buf, narrow_buf)
        cols = (pl.ds(0, n), pl.ds(0, wide), pl.ds(wide, _LANES))

        def start(load, priority):
            which, group, slot, sem = load
            pltpu.make_async_copy(
                x_hbm.at[pl.ds(group * _SUB, _SUB), cols[which]],
                bufs[which].at[pl.ds(slot * _SUB, _SUB)],
                load_sems.at[sem],
            ).start(priority=priority)

        def wait(buf, slot, count, sem):
            filled = buf.at[pl.ds(slot * _SUB, count * _SUB)]
            pltpu.make_async_copy(filled, filled, load_sems.at[sem]).wait()

        for ld, priority in starts[:_PREFILL]:
            start(ld, priority)

        peer = (1 - lax.axis_index("x"), lax.axis_index("y"))
        barrier = pltpu.get_barrier_semaphore()
        pl.semaphore_signal(barrier, inc=1, device_id=peer, device_id_type=pl.DeviceIdType.MESH)

        for ld, priority in starts[_PREFILL:]:
            start(ld, priority)
        pl.semaphore_wait(barrier, 1)

        def exchange(i, lanes):
            return pltpu.make_async_remote_copy(
                src_ref=mine.at[:, lanes],
                dst_ref=theirs.at[:, lanes],
                send_sem=send_sems.at[i],
                recv_sem=recv_sems.at[i],
                device_id=peer,
                device_id_type=pl.DeviceIdType.MESH,
            )

        def group(buf, slot):
            return buf[pl.ds(slot * _SUB, _SUB), :]

        sem = 0
        slot = 0
        acc = jnp.zeros((_SUB, n), jnp.float32)
        for count in full_parts:
            wait(full_buf, slot, count, sem)

            def step(i, acc, slot=slot):
                row = pl.multiple_of((slot + i * _UNROLL) * _SUB, _SUB)
                block = full_buf[pl.ds(row, _UNROLL * _SUB), :]
                for u in range(_UNROLL):
                    acc = acc + block[u * _SUB:(u + 1) * _SUB]
                return acc

            assert count % _UNROLL == 0
            acc = lax.fori_loop(0, count // _UNROLL, step, acc)
            slot += count
            sem += 1

        acc_wide, acc_narrow = acc[:, :wide], acc[:, wide:]
        slot = 0
        for count in wide_parts:
            wait(wide_buf, slot, count, sem)
            acc_wide = acc_wide + _tree_sum(group(wide_buf, slot + u) for u in range(count))
            slot += count
            sem += 1
        mine[:, cols[1]] = jnp.sum(acc_wide, axis=0, keepdims=True)
        first = exchange(0, cols[1])
        first.start()

        slot = 0
        for count in narrow_parts:
            wait(narrow_buf, slot, count, sem)
            acc_narrow = _tree_sum([group(narrow_buf, slot + u) for u in range(count)] + [acc_narrow])
            slot += count
            sem += 1
        mine[:, cols[2]] = jnp.sum(acc_narrow, axis=0, keepdims=True)
        second = exchange(1, cols[2])
        second.start()

        partial = mine[...]
        first.wait_send()
        second.wait_send()
        first.wait_recv()
        second.wait_recv()
        out_ref[...] = partial + theirs[...]

    return pl.pallas_call(
        body,
        out_shape=jax.ShapeDtypeStruct((1, n), jnp.float32),
        in_specs=[pl.BlockSpec(memory_space=pltpu.HBM)],
        out_specs=pl.BlockSpec(memory_space=pltpu.VMEM),
        scratch_shapes=[
            pltpu.VMEM((n_full * _SUB, n), jnp.float32),
            pltpu.VMEM((_TAIL * _SUB, wide), jnp.float32),
            pltpu.VMEM((_TAIL * _SUB, _LANES), jnp.float32),
            pltpu.VMEM((1, n), jnp.float32),
            pltpu.VMEM((1, n), jnp.float32),
            pltpu.SemaphoreType.DMA((n_sems,)),
            pltpu.SemaphoreType.DMA((2,)),
            pltpu.SemaphoreType.DMA((2,)),
        ],
        compiler_params=pltpu.CompilerParams(
            collective_id=0,
            disable_bounds_checks=True,
            disable_semaphore_checks=True,
        ),
    )(x)
```

```python
import jax
import jax.numpy as jnp
from jax import lax
from jax.experimental import pallas as pl
from jax.experimental.pallas import tpu as pltpu

SUBLANES, LANES = 8, 128

ORDER_BASIS = (64, 34, 128, 1, 2, 4, 8, 16)
ORDER_ROTATION = 63
LOW_PRIORITY_LEAD = 28
SPLIT_RUNS = 16
LAST_FULL, LAST_WIDE, LAST_NARROW = 24, 2, 2
RUNS_PER_LOOP_STEP = 8


def _read_order(n_runs):
    order = []
    for step in range(n_runs):
        run = 0
        for bit, vector in enumerate(ORDER_BASIS):
            if (step >> bit) & 1:
                run ^= vector
        order.append((run - ORDER_ROTATION) % n_runs)
    assert sorted(order) == list(range(n_runs))
    return order


def _plan_reads(n_groups, n_blocks):
    order = [u for u in _read_order(n_groups) if u]
    whole, split = order[:-SPLIT_RUNS], order[-SPLIT_RUNS:]
    full = [u * n_blocks - 1 for u in whole]
    wide = [0] + [u * n_blocks for u in split]
    narrow = [n_groups * n_blocks - 1] + [u * n_blocks - 1 for u in split]

    stages, reads = [], []
    for firsts, tiles, last in (
        (full, n_blocks, LAST_FULL),
        (wide, n_blocks - 1, LAST_WIDE),
        (narrow, 1, LAST_NARROW),
    ):
        for part in (firsts[:-last], firsts[-last:]):
            reads += [(len(stages), slot, first) for slot, first in enumerate(part)]
            stages.append((tiles, len(part)))
    covered = [first + i for stage, _, first in reads for i in range(stages[stage][0])]
    assert sorted(covered) == list(range(n_groups * n_blocks))

    pairs = (len(reads) - LOW_PRIORITY_LEAD) // 2
    low = reads[: 2 * pairs : 2] + reads[2 * pairs :]
    high = reads[1 : 2 * pairs : 2]
    starts = [(*read, 1) for read in low[:LOW_PRIORITY_LEAD]]
    for i in range(pairs):
        starts += [(*high[i], 0), (*low[LOW_PRIORITY_LEAD + i], 1)]
    starts += [(*read, 1) for read in low[LOW_PRIORITY_LEAD + pairs :]]
    return stages, starts


def _tree_sum(values):
    while len(values) > 1:
        pairs = [a + b for a, b in zip(values[::2], values[1::2])]
        values = pairs + values[2 * len(pairs) :]
    return values[0]


def pallas_dist_sum_ax0_xy_m2048_n1024_kernel(x: jax.Array):
    m, n = x.shape
    n_groups, n_blocks = m // SUBLANES, n // LANES
    wide = n - LANES
    stages, starts = _plan_reads(n_groups, n_blocks)

    def body(x_hbm, out_ref, landing, mine, theirs, read_sems, send_sems, recv_sems):
        def start_reads(some):
            for stage, slot, first, priority in some:
                rows = stages[stage][0] * SUBLANES
                pltpu.make_async_copy(
                    x_hbm.at[pl.ds(first * SUBLANES, rows)],
                    landing[stage].at[pl.ds(slot * rows, rows)],
                    read_sems.at[stage],
                ).start(priority=priority)

        def landed(stage):
            buf = landing[stage]
            pltpu.make_async_copy(buf, buf, read_sems.at[stage]).wait()
            return buf

        def tile(buf, i):
            return buf[pl.ds(i * SUBLANES, SUBLANES), :]

        start_reads(starts[: 2 * LOW_PRIORITY_LEAD])
        peer = (1 - lax.axis_index("x"), lax.axis_index("y"))
        barrier = pltpu.get_barrier_semaphore()
        pl.semaphore_signal(
            barrier, inc=1, device_id=peer, device_id_type=pl.DeviceIdType.MESH
        )
        start_reads(starts[2 * LOW_PRIORITY_LEAD :])

        sums = (jnp.zeros((SUBLANES, LANES), jnp.float32),) * n_blocks
        for stage in (0, 1):
            buf = landed(stage)
            step_tiles = RUNS_PER_LOOP_STEP * n_blocks
            steps = stages[stage][1] // RUNS_PER_LOOP_STEP

            def add_runs(i, sums, buf=buf):
                rows = step_tiles * SUBLANES
                block = buf[pl.ds(pl.multiple_of(i * rows, rows), rows), :]
                sums = list(sums)
                for t in range(step_tiles):
                    sums[t % n_blocks] += block[t * SUBLANES : (t + 1) * SUBLANES]
                return tuple(sums)

            sums = list(lax.fori_loop(0, steps, add_runs, tuple(sums)))
            for t in range(steps * step_tiles, stages[stage][1] * n_blocks):
                sums[t % n_blocks] += tile(buf, t)
        last_block, other_blocks = sums[0], sums[1:]

        pl.semaphore_wait(barrier, 1)
        swaps = [
            pltpu.make_async_remote_copy(
                src_ref=mine[i],
                dst_ref=theirs[i],
                send_sem=send_sems.at[i],
                recv_sem=recv_sems.at[i],
                device_id=peer,
                device_id_type=pl.DeviceIdType.MESH,
            )
            for i in range(2)
        ]

        for stage in (2, 3):
            buf = landed(stage)
            tiles, count = stages[stage]
            other_blocks = [
                _tree_sum([tile(buf, slot * tiles + j) for slot in range(count)] + [acc])
                for j, acc in enumerate(other_blocks)
            ]
        mine[0][...] = jnp.concatenate(
            [jnp.sum(acc, axis=0, keepdims=True) for acc in other_blocks], axis=1
        )
        swaps[0].start()

        for stage in (4, 5):
            buf = landed(stage)
            last_block = _tree_sum(
                [tile(buf, slot) for slot in range(stages[stage][1])] + [last_block]
            )
        mine[1][...] = jnp.sum(last_block, axis=0, keepdims=True)
        swaps[1].start()

        partial = [ref[...] for ref in mine]
        for swap in swaps:
            swap.wait_send()
        for i, lanes in enumerate((pl.ds(0, wide), pl.ds(wide, LANES))):
            swaps[i].wait_recv()
            out_ref[:, lanes] = partial[i] + theirs[i][...]

    x_tiles = (
        x.reshape(n_groups, SUBLANES, n_blocks, LANES)
        .transpose(0, 2, 1, 3)
        .reshape(n_groups * n_blocks * SUBLANES, LANES)
    )
    messages = [pltpu.VMEM((1, wide), jnp.float32), pltpu.VMEM((1, LANES), jnp.float32)]
    return pl.pallas_call(
        body,
        out_shape=jax.ShapeDtypeStruct((1, n), jnp.float32),
        in_specs=[pl.BlockSpec(memory_space=pltpu.HBM)],
        out_specs=pl.BlockSpec(memory_space=pltpu.VMEM),
        scratch_shapes=[
            [
                pltpu.VMEM((tiles * count * SUBLANES, LANES), jnp.float32)
                for tiles, count in stages
            ],
            messages,
            messages,
            pltpu.SemaphoreType.DMA((len(stages),)),
            pltpu.SemaphoreType.DMA((2,)),
            pltpu.SemaphoreType.DMA((2,)),
        ],
        compiler_params=pltpu.CompilerParams(
            collective_id=0,
            disable_semaphore_checks=True,
        ),
    )(x_tiles)
```
